```python
import numpy as np

kernel_name = "dist_argmax_global_i_m4096_n1024"

def setup_inputs():
    return {"x": np.random.randn(16384, 1024).astype(np.float32)}

def reference(x: np.ndarray) -> np.ndarray:
    idx = np.argmax(x, axis=0).astype(np.float32)
    val = np.max(x, axis=0)
    return np.stack([val, idx], axis=0)
```

```python
import functools

import jax
import jax.numpy as jnp
from jax import lax
from jax.experimental import pallas as pl
from jax.experimental.pallas import tpu as pltpu

N_DEV = 4
BM = 512
SUB = 8


def pallas_dist_argmax_global_i_m4096_n1024_kernel(
    x: jax.Array,
):
    m_per, n = x.shape
    nb = m_per // BM
    assert m_per % BM == 0 and BM % SUB == 0

    def body(x_ref, out_ref, m_ref, g_ref, comm_ref, send_sems, recv_sems):
        step = pl.program_id(0)
        my = lax.axis_index("i")

        @pl.when(step == 0)
        def _():
            bsem = pltpu.get_barrier_semaphore()
            for d in range(1, N_DEV):
                pl.semaphore_signal(
                    bsem, inc=1, device_id=((my + d) % N_DEV,),
                    device_id_type=pl.DeviceIdType.MESH,
                )
            m_ref[...] = jnp.full((SUB, n), -jnp.inf, jnp.float32)
            g_ref[...] = jnp.zeros((SUB, n), jnp.int32)

        m = m_ref[...]
        g = g_ref[...]
        base = step * (BM // SUB)
        for k in range(BM // SUB):
            v = x_ref[pl.ds(k * SUB, SUB), :]
            gt = v > m
            m = jnp.where(gt, v, m)
            g = jnp.where(gt, base + k, g)
        m_ref[...] = m
        g_ref[...] = g

        @pl.when(step == nb - 1)
        def _():
            row = g * SUB + lax.broadcasted_iota(jnp.int32, (SUB, n), 0) + my * m_per
            best = jnp.max(m, axis=0, keepdims=True)
            cand = jnp.where(m == best, row, jnp.int32(2**30))
            bidx = jnp.min(cand, axis=0, keepdims=True).astype(jnp.float32)
            comm_ref[my, 0:1, :] = best
            comm_ref[my, 1:2, :] = bidx

            bsem = pltpu.get_barrier_semaphore()
            pl.semaphore_wait(bsem, N_DEV - 1)

            copies = []
            for d in range(1, N_DEV):
                peer = (my + d) % N_DEV
                cp = pltpu.make_async_remote_copy(
                    src_ref=comm_ref.at[my],
                    dst_ref=comm_ref.at[my],
                    send_sem=send_sems.at[d - 1],
                    recv_sem=recv_sems.at[d - 1],
                    device_id=(peer,),
                    device_id_type=pl.DeviceIdType.MESH,
                )
                cp.start()
                copies.append(cp)
            for cp in copies:
                cp.wait()

            val = comm_ref[0, 0:1, :]
            idx = comm_ref[0, 1:2, :]
            for k in range(1, N_DEV):
                vk = comm_ref[k, 0:1, :]
                ik = comm_ref[k, 1:2, :]
                gt = vk > val
                val = jnp.where(gt, vk, val)
                idx = jnp.where(gt, ik, idx)
            out_ref[0:1, :] = val
            out_ref[1:2, :] = idx

    return pl.pallas_call(
        body,
        out_shape=jax.ShapeDtypeStruct((2, n), jnp.float32),
        grid=(nb,),
        in_specs=[pl.BlockSpec((BM, n), lambda i: (i, 0))],
        out_specs=pl.BlockSpec((2, n), lambda i: (0, 0)),
        scratch_shapes=[
            pltpu.VMEM((SUB, n), jnp.float32),
            pltpu.VMEM((SUB, n), jnp.int32),
            pltpu.VMEM((N_DEV, 2, n), jnp.float32),
            pltpu.SemaphoreType.DMA((N_DEV - 1,)),
            pltpu.SemaphoreType.DMA((N_DEV - 1,)),
        ],
        compiler_params=pltpu.CompilerParams(
            collective_id=0, dimension_semantics=("arbitrary",)
        ),
    )(x)
```

```python
import jax
import jax.numpy as jnp
from jax import lax
from jax.experimental import pallas as pl
from jax.experimental.pallas import tpu as pltpu

N_DEV = 4
SUB = 8


def _chunks(m_per):
    sizes, left = [], m_per
    while left > 1024:
        sizes.append(512)
        left -= 512
    while left > 64:
        sizes.append(left // 2)
        left -= left // 2
    sizes.append(left)
    starts = [sum(sizes[:i]) for i in range(len(sizes))]
    return list(zip(starts, sizes))


def _better(v, m):
    return jnp.logical_or(v > m, jnp.logical_and(v != v, m == m))


def pallas_dist_argmax_global_i_m4096_n1024_kernel(
    x: jax.Array,
):
    m_per, n = x.shape
    chunks = _chunks(m_per)
    nch = len(chunks)

    def body(x_hbm, out_ref, buf, comm_ref, dsems, send_sems, recv_sems):
        my = lax.axis_index("i")
        copies = []
        for c, (s, sz) in enumerate(chunks):
            cp = pltpu.make_async_copy(
                x_hbm.at[pl.ds(s, sz), :], buf.at[pl.ds(s, sz), :], dsems.at[c]
            )
            cp.start()
            copies.append(cp)

        bsem = pltpu.get_barrier_semaphore()
        for d in range(1, N_DEV):
            pl.semaphore_signal(
                bsem, inc=1, device_id=((my + d) % N_DEV,),
                device_id_type=pl.DeviceIdType.MESH,
            )

        m = jnp.full((SUB, n), -jnp.inf, jnp.float32)
        g = jnp.zeros((SUB, n), jnp.int32)
        for c, (s, sz) in enumerate(chunks):
            copies[c].wait()

            def inner(k, carry, s=s):
                m, g = carry
                r = s // SUB + k
                v = buf[pl.ds(pl.multiple_of(r * SUB, SUB), SUB), :]
                gt = _better(v, m)
                return jnp.where(gt, v, m), jnp.where(gt, r, g)

            m, g = lax.fori_loop(0, sz // SUB, inner, (m, g), unroll=8)

        row = g * SUB + lax.broadcasted_iota(jnp.int32, (SUB, n), 0) + my * m_per
        best = jnp.max(m, axis=0, keepdims=True)
        cand = jnp.where(jnp.logical_or(m == best, m != m), row, jnp.int32(2**30))
        bidx = jnp.min(cand, axis=0, keepdims=True).astype(jnp.float32)
        comm_ref[my, 0:1, :] = best
        comm_ref[my, 1:2, :] = bidx

        pl.semaphore_wait(bsem, N_DEV - 1)

        rcs = []
        for d in range(1, N_DEV):
            peer = (my + d) % N_DEV
            cp = pltpu.make_async_remote_copy(
                src_ref=comm_ref.at[my],
                dst_ref=comm_ref.at[my],
                send_sem=send_sems.at[d - 1],
                recv_sem=recv_sems.at[d - 1],
                device_id=(peer,),
                device_id_type=pl.DeviceIdType.MESH,
            )
            cp.start()
            rcs.append(cp)
        for cp in rcs:
            cp.wait()

        val = comm_ref[0, 0:1, :]
        idx = comm_ref[0, 1:2, :]
        for k in range(1, N_DEV):
            vk = comm_ref[k, 0:1, :]
            ik = comm_ref[k, 1:2, :]
            gt = _better(vk, val)
            val = jnp.where(gt, vk, val)
            idx = jnp.where(gt, ik, idx)
        out_ref[0:1, :] = val
        out_ref[1:2, :] = idx

    return pl.pallas_call(
        body,
        out_shape=jax.ShapeDtypeStruct((2, n), jnp.float32),
        in_specs=[pl.BlockSpec(memory_space=pl.ANY)],
        out_specs=pl.BlockSpec(memory_space=pltpu.VMEM),
        scratch_shapes=[
            pltpu.VMEM((m_per, n), jnp.float32),
            pltpu.VMEM((N_DEV, 2, n), jnp.float32),
            pltpu.SemaphoreType.DMA((nch,)),
            pltpu.SemaphoreType.DMA((N_DEV - 1,)),
            pltpu.SemaphoreType.DMA((N_DEV - 1,)),
        ],
        compiler_params=pltpu.CompilerParams(
            collective_id=0, vmem_limit_bytes=64 * 1024 * 1024
        ),
    )(x)
```
